```python
import numpy as np

kernel_name = "dist_mean_ax1_xy_m1024_n512"

def setup_inputs():
    return {"x": np.random.randn(2048, 1024).astype(np.float32)}

def reference(x: np.ndarray) -> np.ndarray:
    return np.mean(x, axis=1, keepdims=True)
```

```python
import jax
import jax.numpy as jnp
from jax import lax
from jax.experimental import pallas as pl
from jax.experimental.pallas import tpu as pltpu

LANES = 128
SUBLANES = 8
Y_SIZE = 2

CHUNKS = (256, 256, 256, 128, 80, 48)
SENDS = (7, 1)


def pallas_dist_mean_ax1_xy_m1024_n512_kernel(x: jax.Array):
    m, n = x.shape
    n_global = Y_SIZE * n
    nb = m // LANES
    assert sum(CHUNKS) == m and sum(SENDS) == nb and n % LANES == 0

    def body(x_hbm, out_ref, xbuf, send_buf, recv_buf, load_sems, send_sems, recv_sems):
        my_x = lax.axis_index("x")
        my_y = lax.axis_index("y")
        nbr = (my_x, 1 - my_y)

        loads = []
        off = 0
        for i, c in enumerate(CHUNKS):
            cp = pltpu.make_async_copy(
                x_hbm.at[pl.ds(off, c)], xbuf.at[pl.ds(off, c)], load_sems.at[i])
            cp.start()
            loads.append((off, c, cp))
            off += c

        bsem = pltpu.get_barrier_semaphore()
        pl.semaphore_signal(bsem, inc=1, device_id=nbr,
                            device_id_type=pl.DeviceIdType.MESH)

        send_at = {}
        b0 = 0
        for k, s in enumerate(SENDS):
            send_at[b0 + s - 1] = (k, b0, s)
            b0 += s

        def diag8(r0, r):
            xb = xbuf[pl.ds(r0, r), :]
            parts = [xb[:, j * LANES:(j + 1) * LANES] for j in range(n // LANES)]
            while len(parts) > 1:
                parts = [parts[j] + parts[j + 1] if j + 1 < len(parts) else parts[j]
                         for j in range(0, len(parts), 2)]
            s = jnp.sum(parts[0], axis=1, keepdims=True)
            row = lax.broadcasted_iota(jnp.int32, (r, LANES), 0) + (r0 % LANES)
            lane = lax.broadcasted_iota(jnp.int32, (r, LANES), 1)
            d = jnp.where(row == lane, s, 0.0)
            acc = d[0:SUBLANES]
            for g in range(1, r // SUBLANES):
                acc = acc + d[SUBLANES * g:SUBLANES * (g + 1)]
            return acc

        rdmas = []
        acc = None
        for off, c, cp in loads:
            cp.wait()
            r0, end = off, off + c
            while r0 < end:
                b = r0 // LANES
                r = min(end, (b + 1) * LANES) - r0
                d = diag8(r0, r)
                acc = d if acc is None else acc + d
                r0 += r
                if r0 % LANES:
                    continue
                send_buf[b] = jnp.sum(acc, axis=0, keepdims=True)
                acc = None
                if b in send_at:
                    k, sb0, sn = send_at[b]
                    if k == 0:
                        pl.semaphore_wait(bsem, 1)
                    rdma = pltpu.make_async_remote_copy(
                        src_ref=send_buf.at[pl.ds(sb0, sn)],
                        dst_ref=recv_buf.at[pl.ds(sb0, sn)],
                        send_sem=send_sems.at[k], recv_sem=recv_sems.at[k],
                        device_id=nbr, device_id_type=pl.DeviceIdType.MESH)
                    rdma.start()
                    rdmas.append((rdma, sb0, sn))

        for rdma, _, _ in rdmas:
            rdma.wait_send()
        for rdma, sb0, sn in rdmas:
            rdma.wait_recv()
            rows = pl.ds(sb0, sn)
            out_ref[rows] = (send_buf[rows] + recv_buf[rows]) * (1.0 / n_global)

    out = pl.pallas_call(
        body,
        out_shape=jax.ShapeDtypeStruct((nb, 1, LANES), jnp.float32),
        in_specs=[pl.BlockSpec(memory_space=pl.ANY)],
        out_specs=pl.BlockSpec(memory_space=pltpu.VMEM),
        scratch_shapes=[
            pltpu.VMEM((m, n), jnp.float32),
            pltpu.VMEM((nb, 1, LANES), jnp.float32),
            pltpu.VMEM((nb, 1, LANES), jnp.float32),
            pltpu.SemaphoreType.DMA((len(CHUNKS),)),
            pltpu.SemaphoreType.DMA((len(SENDS),)),
            pltpu.SemaphoreType.DMA((len(SENDS),)),
        ],
        compiler_params=pltpu.CompilerParams(
            collective_id=0, disable_bounds_checks=True, disable_semaphore_checks=True),
    )(x)
    return out.reshape(m, 1)
```

```python
import jax
import jax.numpy as jnp
from jax import lax
from jax.experimental import pallas as pl
from jax.experimental.pallas import tpu as pltpu

LANES = 128
SUBLANES = 8
Y_SIZE = 2

CHUNKS = (256, 256, 256, 128, 80)
RAW_ROWS = 48

EARLY, LATE, TAIL, RAW = range(4)


def pallas_dist_mean_ax1_xy_m1024_n512_kernel(x: jax.Array):
    m, n = x.shape
    nb = m // LANES
    main = m - RAW_ROWS
    assert sum(CHUNKS) == main and (nb - 1) * LANES < main < m and n % LANES == 0
    scale = 1.0 / (Y_SIZE * n)
    mesh_id = pl.DeviceIdType.MESH

    def body(x_hbm, out_ref, xbuf, rawbuf, send_buf, recv_buf,
             load_sems, send_sems, recv_sems):
        my_y = lax.axis_index("y")
        nbr = (lax.axis_index("x"), 1 - my_y)

        def load(i, r0, r):
            rows = pl.ds(r0, r)
            return pltpu.make_async_copy(x_hbm.at[rows], xbuf.at[rows], load_sems.at[i])

        def to_nbr(k, src, dst):
            return pltpu.make_async_remote_copy(
                src_ref=src, dst_ref=dst,
                send_sem=send_sems.at[k], recv_sem=recv_sems.at[k],
                device_id=nbr, device_id_type=mesh_id)

        def partials(k, b0, cnt):
            rows = pl.ds(b0, cnt)
            return to_nbr(k, send_buf.at[rows], recv_buf.at[rows])

        def row_sums(ref, r0, r, lane0):
            xb = ref[pl.ds(r0, r), :]
            parts = [xb[:, j * LANES:(j + 1) * LANES] for j in range(n // LANES)]
            while len(parts) > 1:
                parts = [parts[j] + parts[j + 1] if j + 1 < len(parts) else parts[j]
                         for j in range(0, len(parts), 2)]
            s = jnp.sum(parts[0], axis=1, keepdims=True)
            row = lax.broadcasted_iota(jnp.int32, (r, LANES), 0) + lane0
            lane = lax.broadcasted_iota(jnp.int32, (r, LANES), 1)
            d = jnp.where(row == lane, s, 0.0)
            acc = d[0:SUBLANES]
            for g in range(1, r // SUBLANES):
                acc = acc + d[SUBLANES * g:SUBLANES * (g + 1)]
            return jnp.sum(acc, axis=0, keepdims=True)

        loads = []
        r0 = 0
        for i, r in enumerate(CHUNKS):
            loads.append((r0, r, load(i, r0, r)))
            loads[-1][2].start()
            r0 += r
        tail_load = load(len(CHUNKS), main, RAW_ROWS)

        early = partials(EARLY, 0, nb - 1)
        late = partials(LATE, nb - 1, 1)
        tail = partials(TAIL, nb, 1)
        raw = to_nbr(RAW, x_hbm.at[pl.ds(main, RAW_ROWS)], rawbuf)

        barrier = pltpu.get_barrier_semaphore()
        pl.semaphore_signal(barrier, inc=1, device_id=nbr, device_id_type=mesh_id)

        @pl.when(my_y == 1)
        def _():
            pl.semaphore_wait(barrier, 1)
            raw.start()

        @pl.when(my_y == 0)
        def _():
            tail_load.start()

        for r0, r, cp in loads:
            cp.wait()
            assert r0 % LANES == 0
            for q0 in range(r0, r0 + r, LANES):
                b = q0 // LANES
                send_buf[b] = row_sums(xbuf, q0, min(LANES, r0 + r - q0), 0)
                if b == nb - 2:
                    @pl.when(my_y == 0)
                    def _():
                        pl.semaphore_wait(barrier, 1)
                    early.start()
                if b == nb - 1:
                    late.start()

        @pl.when(my_y == 1)
        def _():
            tail_load.start()

        tail_load.wait()
        send_buf[nb] = row_sums(xbuf, main, RAW_ROWS, main % LANES)

        @pl.when(my_y == 0)
        def _():
            tail.start()
            raw.wait_recv()
            recv_buf[nb] = row_sums(rawbuf, 0, RAW_ROWS, main % LANES)
            tail.wait_send()

        @pl.when(my_y == 1)
        def _():
            raw.wait_send()
            tail.wait_recv()

        early.wait_send()
        late.wait_send()
        last = send_buf[nb - 1] + send_buf[nb] + recv_buf[nb]
        early.wait_recv()
        rows = pl.ds(0, nb - 1)
        out_ref[rows] = (send_buf[rows] + recv_buf[rows]) * scale
        late.wait_recv()
        out_ref[nb - 1] = (last + recv_buf[nb - 1]) * scale

    out = pl.pallas_call(
        body,
        out_shape=jax.ShapeDtypeStruct((nb, 1, LANES), jnp.float32),
        in_specs=[pl.BlockSpec(memory_space=pl.ANY)],
        out_specs=pl.BlockSpec(memory_space=pltpu.VMEM),
        scratch_shapes=[
            pltpu.VMEM((m, n), jnp.float32),
            pltpu.VMEM((RAW_ROWS, n), jnp.float32),
            pltpu.VMEM((nb + 1, 1, LANES), jnp.float32),
            pltpu.VMEM((nb + 1, 1, LANES), jnp.float32),
            pltpu.SemaphoreType.DMA((len(CHUNKS) + 1,)),
            pltpu.SemaphoreType.DMA((4,)),
            pltpu.SemaphoreType.DMA((4,)),
        ],
        compiler_params=pltpu.CompilerParams(
            collective_id=0, disable_bounds_checks=True, disable_semaphore_checks=True),
    )(x)
    return out.reshape(m, 1)
```

```python
import jax
import jax.numpy as jnp
from jax import lax
from jax.experimental import pallas as pl
from jax.experimental.pallas import tpu as pltpu

LANES = 128
SUBLANES = 8
Y_SIZE = 2

CHUNKS = (256, 256, 256, 128, 80)
RAW_ROWS = 48

EARLY, LATE, TAIL, RAW = range(4)


def _compiler_params():
    try:
        return pltpu.CompilerParams(
            collective_id=0, disable_bounds_checks=True, disable_semaphore_checks=True)
    except TypeError:
        return pltpu.CompilerParams(collective_id=0, disable_bounds_checks=True)


def pallas_dist_mean_ax1_xy_m1024_n512_kernel(x: jax.Array):
    m, n = x.shape
    nb = m // LANES
    main = m - RAW_ROWS
    assert sum(CHUNKS) == main and (nb - 1) * LANES < main < m and n % LANES == 0
    scale = 1.0 / (Y_SIZE * n)
    mesh_id = pl.DeviceIdType.MESH

    def body(x_hbm, out_ref, xbuf, rawbuf, send_buf, recv_buf,
             load_sems, send_sems, recv_sems):
        my_y = lax.axis_index("y")
        nbr = (lax.axis_index("x"), 1 - my_y)

        def load(i, r0, r):
            rows = pl.ds(r0, r)
            return pltpu.make_async_copy(x_hbm.at[rows], xbuf.at[rows], load_sems.at[i])

        def to_nbr(k, src, dst):
            return pltpu.make_async_remote_copy(
                src_ref=src, dst_ref=dst,
                send_sem=send_sems.at[k], recv_sem=recv_sems.at[k],
                device_id=nbr, device_id_type=mesh_id)

        def partials(k, b0, cnt):
            rows = pl.ds(b0, cnt)
            return to_nbr(k, send_buf.at[rows], recv_buf.at[rows])

        def row_sums(ref, r0, r, lane0):
            xb = ref[pl.ds(r0, r), :]
            parts = [xb[:, j * LANES:(j + 1) * LANES] for j in range(n // LANES)]
            while len(parts) > 1:
                parts = [parts[j] + parts[j + 1] if j + 1 < len(parts) else parts[j]
                         for j in range(0, len(parts), 2)]
            s = jnp.sum(parts[0], axis=1, keepdims=True)
            row = lax.broadcasted_iota(jnp.int32, (r, LANES), 0) + lane0
            lane = lax.broadcasted_iota(jnp.int32, (r, LANES), 1)
            d = jnp.where(row == lane, s, 0.0)
            acc = d[0:SUBLANES]
            for g in range(1, r // SUBLANES):
                acc = acc + d[SUBLANES * g:SUBLANES * (g + 1)]
            return jnp.sum(acc, axis=0, keepdims=True)

        loads = []
        r0 = 0
        for i, r in enumerate(CHUNKS):
            loads.append((r0, r, load(i, r0, r)))
            loads[-1][2].start()
            r0 += r
        tail_load = load(len(CHUNKS), main, RAW_ROWS)

        early = partials(EARLY, 0, nb - 1)
        late = partials(LATE, nb - 1, 1)
        tail = partials(TAIL, nb, 1)
        raw = to_nbr(RAW, x_hbm.at[pl.ds(main, RAW_ROWS)], rawbuf)

        barrier = pltpu.get_barrier_semaphore()
        pl.semaphore_signal(barrier, inc=1, device_id=nbr, device_id_type=mesh_id)

        @pl.when(my_y == 1)
        def _():
            pl.semaphore_wait(barrier, 1)
            raw.start()

        @pl.when(my_y == 0)
        def _():
            tail_load.start()

        for r0, r, cp in loads:
            cp.wait()
            assert r0 % LANES == 0
            for q0 in range(r0, r0 + r, LANES):
                b = q0 // LANES
                send_buf[b] = row_sums(xbuf, q0, min(LANES, r0 + r - q0), 0)
                if b == nb - 2:
                    @pl.when(my_y == 0)
                    def _():
                        pl.semaphore_wait(barrier, 1)
                    early.start()
                if b == nb - 1:
                    late.start()

        @pl.when(my_y == 1)
        def _():
            tail_load.start()

        tail_load.wait()
        send_buf[nb] = row_sums(xbuf, main, RAW_ROWS, main % LANES)

        @pl.when(my_y == 0)
        def _():
            tail.start()
            raw.wait_recv()
            recv_buf[nb] = row_sums(rawbuf, 0, RAW_ROWS, main % LANES)
            tail.wait_send()

        @pl.when(my_y == 1)
        def _():
            raw.wait_send()
            tail.wait_recv()

        early.wait_send()
        late.wait_send()
        last = send_buf[nb - 1] + send_buf[nb] + recv_buf[nb]
        early.wait_recv()
        rows = pl.ds(0, nb - 1)
        out_ref[rows] = (send_buf[rows] + recv_buf[rows]) * scale
        late.wait_recv()
        out_ref[nb - 1] = (last + recv_buf[nb - 1]) * scale

    out = pl.pallas_call(
        body,
        out_shape=jax.ShapeDtypeStruct((nb, 1, LANES), jnp.float32),
        in_specs=[pl.BlockSpec(memory_space=pl.ANY)],
        out_specs=pl.BlockSpec(memory_space=pltpu.VMEM),
        scratch_shapes=[
            pltpu.VMEM((m, n), jnp.float32),
            pltpu.VMEM((RAW_ROWS, n), jnp.float32),
            pltpu.VMEM((nb + 1, 1, LANES), jnp.float32),
            pltpu.VMEM((nb + 1, 1, LANES), jnp.float32),
            pltpu.SemaphoreType.DMA((len(CHUNKS) + 1,)),
            pltpu.SemaphoreType.DMA((4,)),
            pltpu.SemaphoreType.DMA((4,)),
        ],
        compiler_params=_compiler_params(),
    )(x)
    return out.reshape(m, 1)
```
